```python
import numpy as np

kernel_name = "dist_matmul_mk_i_outk_m1024_n1024_k512"

def setup_inputs():
    A = np.random.randn(1024, 2048).astype(np.float32)
    B = np.random.randn(2048, 1024).astype(np.float32)
    return {"A": A, "B": B}

def reference(A: np.ndarray, B: np.ndarray) -> np.ndarray:
    return A @ B
```

```python
import contextlib
import jax
import jax.numpy as jnp
from jax import lax
from jax.experimental import pallas as pl
from jax.experimental.pallas import tpu as pltpu

N_DEV = 4
M, K, N = 1024, 512, 1024
MB = M // N_DEV
F32, BF16 = jnp.float32, jnp.bfloat16


def make(swing=0, scoped=False, nosem=True, out_dtype=BF16, btiles=(128, 128, 128, 128, 256, 256), first=64, last=16, nobounds=False):
    lo, hi = MB // 2 - swing, MB // 2 + swing
    ns = jax.named_scope if scoped else (lambda n: contextlib.nullcontext())
    cols = []
    c = 0
    for w in btiles:
        cols.append((c, w)); c += w
    assert c == N

    def body(a_hbm, b_hbm, o_ref, a32, b32, a16, b16, sbuf, hop, fin, acc, lsem, ssem, rsem):
        me = lax.axis_index("i")
        right = lax.rem(me + 1, N_DEV)
        diag = lax.rem(me + 2, N_DEV)
        left = lax.rem(me + 3, N_DEV)
        D, R, L, S = 0, 1, 2, 3
        owner = (diag, right, left, me)

        def load_a(blk, r0, nr, s):
            return pltpu.async_copy(a_hbm.at[pl.ds(pl.multiple_of(owner[blk] * MB + r0, 8), nr)], a32.at[blk, pl.ds(r0, nr)], lsem.at[s])

        def load_b(t, s):
            sl = pl.ds(*cols[t])
            return pltpu.async_copy(b_hbm.at[:, sl], b32.at[:, sl], lsem.at[s])

        nb = len(cols)
        ld_b = [None] * nb
        ld_b[0] = load_b(0, 0)
        ld_d1 = [load_a(D, 0, first, nb), load_a(D, MB - first, first, nb)]
        barrier = pltpu.get_barrier_semaphore()
        for nbr in (left, right):
            pl.semaphore_signal(barrier, inc=1, device_id=(nbr,), device_id_type=pl.DeviceIdType.MESH)
        ld_b[1] = load_b(1, 1)
        ld_d2 = load_a(D, first, MB - 2 * first, nb + 1)
        for t in range(2, nb):
            ld_b[t] = load_b(t, t)
        ld_p2 = [load_a(R, hi, MB - hi, nb + 2), load_a(L, 0, lo, nb + 2)]
        ld_s = load_a(S, 0, MB, nb + 3)
        ld_p3 = [load_a(R, 0, hi, nb + 4), load_a(L, lo, MB - lo, nb + 4)]

        FROM_L, FROM_R = 0, 1

        def send(blk, r0, nr, c0, nc, dst, side, sem):
            rs, cs = pl.ds(r0, nr), pl.ds(c0, nc)
            if isinstance(side, int):
                dev = right if side == FROM_L else left
            else:
                dev = jnp.where(side == FROM_L, right, left)
            pltpu.make_async_remote_copy(sbuf.at[blk, rs, cs], dst.at[side, rs, cs], ssem, rsem.at[sem + side],
                                         device_id=(dev,), device_id_type=pl.DeviceIdType.MESH).start()

        def wait(ref, sem):
            pltpu.make_async_copy(ref, ref, sem).wait()

        def cast_b(t):
            sl = pl.ds(*cols[t])
            v = b32[:, sl].astype(BF16)
            b16[:, sl] = v
            return v

        def dot(x, y):
            return jnp.dot(x, y, preferred_element_type=F32)

        HOP, BULK, LAST = 0, 2, 4
        with ns("z_b0"):
            ld_b[0].wait()
        bt = cast_b(0)
        with ns("z_d1"):
            for cp in ld_d1: cp.wait()
        x = jnp.concatenate([a32[D, :first], a32[D, MB - first:]], axis=0).astype(BF16)
        a16[:first] = x[:first]
        a16[MB - first:] = x[first:]
        for t in (0, 1):
            c0, w = cols[t]
            if t == 1:
                with ns("z_b1"):
                    ld_b[1].wait()
                bt = cast_b(1)
                x = jnp.concatenate([a16[:first], a16[MB - first:]], axis=0)
            y = dot(x, bt).astype(BF16)
            sbuf[D, :first, c0:c0 + w] = y[:first]
            sbuf[D, MB - first:, c0:c0 + w] = y[first:]
            if t == 0:
                with ns("z_bar"):
                    pl.semaphore_wait(barrier, 2)
            with ns(f"z_snd{t}"):
                send(D, 0, first, c0, w, hop, FROM_L, HOP)
                send(D, MB - first, first, c0, w, hop, FROM_R, HOP)
        with ns("z_d2"):
            ld_d2.wait()
        w01 = cols[2][0]
        x = a32[D, first:MB - first].astype(BF16)
        a16[first:MB - first] = x
        sbuf[D, first:MB - first, :w01] = dot(x, b16[:, :w01]).astype(BF16)
        with ns("z_snd2"):
            send(D, first, lo - first, 0, w01, hop, FROM_L, HOP)
            send(D, hi, lo - first, 0, w01, hop, FROM_R, HOP)
        for t in range(2, nb):
            c0, w = cols[t]
            with ns(f"z_b{t}"):
                ld_b[t].wait()
            sbuf[D, :, c0:c0 + w] = dot(a16[...], cast_b(t)).astype(BF16)
            with ns(f"z_snd{t+1}"):
                send(D, 0, lo, c0, w, hop, FROM_L, HOP)
                send(D, hi, lo, c0, w, hop, FROM_R, HOP)
        if swing:
            send(D, lo, swing, 0, N, hop, jnp.where(me == 3, FROM_R, FROM_L), HOP)
            send(D, MB // 2, swing, 0, N, hop, jnp.where(me == 1, FROM_L, FROM_R), HOP)

        with ns("z_p2"):
            for cp in ld_p2: cp.wait()
        x = jnp.concatenate([a32[R, hi:], a32[L, :lo]], axis=0).astype(BF16)
        y = dot(x, b16[...]).astype(BF16)
        sbuf[R, hi:] = y[:lo]
        sbuf[L, :lo] = y[lo:]
        with ns("z_snd_p2"):
            send(R, hi, lo, 0, N, fin, FROM_L, BULK)
            send(L, 0, lo, 0, N, fin, FROM_R, BULK)

        with ns("z_own"):
            ld_s.wait()
        acc[...] = dot(a32[S].astype(BF16), b16[...])

        with ns("z_p3"):
            for cp in ld_p3: cp.wait()
        with ns("z_hop"):
            if swing:
                n_rows = jnp.where(me == 0, lo, jnp.where(me == 2, hi, MB // 2))
                for n in (lo, MB // 2, hi):
                    @pl.when(n_rows == n)
                    def _():
                        wait(hop.at[FROM_L, pl.ds(0, n)], rsem.at[HOP + FROM_L])
                        wait(hop.at[FROM_R, pl.ds(MB - n, n)], rsem.at[HOP + FROM_R])
                        if n < hi:
                            hop[FROM_L, n:hi] = jnp.zeros((hi - n, N), BF16)
                            hop[FROM_R, lo:MB - n] = jnp.zeros((hi - n, N), BF16)
            else:
                wait(hop.at[FROM_L, pl.ds(0, lo)], rsem.at[HOP + FROM_L])
                wait(hop.at[FROM_R, pl.ds(lo, lo)], rsem.at[HOP + FROM_R])
        x = jnp.concatenate([a32[R, :hi], a32[L, lo:]], axis=0).astype(BF16)
        y = dot(x, b16[...])
        sbuf[R, :hi] = (y[:hi] + hop[FROM_L, :hi].astype(F32)).astype(BF16)
        sbuf[L, lo:] = (y[hi:] + hop[FROM_R, lo:].astype(F32)).astype(BF16)
        with ns("z_snd_p3"):
            send(R, last, hi - last, 0, N, fin, FROM_L, BULK)
            send(L, lo, hi - last, 0, N, fin, FROM_R, BULK)
            send(R, 0, last, 0, N, fin, FROM_L, LAST)
            send(L, MB - last, last, 0, N, fin, FROM_R, LAST)

        with ns("z_bulk"):
            wait(fin.at[FROM_L, pl.ds(last, MB - last)], rsem.at[BULK + FROM_L])
            wait(fin.at[FROM_R, pl.ds(0, MB - last)], rsem.at[BULK + FROM_R])
        mid = slice(last, MB - last)
        o_ref[mid] = (acc[mid] + fin[FROM_L, mid].astype(F32) + fin[FROM_R, mid].astype(F32)).astype(o_ref.dtype)
        acc[:last] += fin[FROM_R, :last].astype(F32)
        acc[MB - last:] += fin[FROM_L, MB - last:].astype(F32)
        with ns("z_sent"):
            wait(sbuf, ssem)
        with ns("z_lastL"):
            wait(fin.at[FROM_L, pl.ds(0, last)], rsem.at[LAST + FROM_L])
        o_ref[:last] = (acc[:last] + fin[FROM_L, :last].astype(F32)).astype(o_ref.dtype)
        with ns("z_lastR"):
            wait(fin.at[FROM_R, pl.ds(MB - last, last)], rsem.at[LAST + FROM_R])
        o_ref[MB - last:] = (acc[MB - last:] + fin[FROM_R, MB - last:].astype(F32)).astype(o_ref.dtype)

    def fn(A, B):
        return pl.pallas_call(
            body,
            out_shape=jax.ShapeDtypeStruct((MB, N), out_dtype),
            in_specs=[pl.BlockSpec(memory_space=pl.ANY)] * 2,
            out_specs=pl.BlockSpec(memory_space=pltpu.VMEM),
            scratch_shapes=[
                pltpu.VMEM((N_DEV, MB, K), F32), pltpu.VMEM((K, N), F32),
                pltpu.VMEM((MB, K), BF16), pltpu.VMEM((K, N), BF16),
                pltpu.VMEM((3, MB, N), BF16), pltpu.VMEM((2, MB, N), BF16), pltpu.VMEM((2, MB, N), BF16),
                pltpu.VMEM((MB, N), F32),
                pltpu.SemaphoreType.DMA((len(cols) + 5,)), pltpu.SemaphoreType.DMA, pltpu.SemaphoreType.DMA((6,)),
            ],
            compiler_params=pltpu.CompilerParams(collective_id=0, disable_semaphore_checks=nosem, disable_bounds_checks=nobounds),
        )(A, B)
    return fn


def pallas_dist_matmul_mk_i_outk_m1024_n1024_k512_kernel(A: jax.Array, B: jax.Array):
    return make(btiles=(128,) * 8)(A, B)
```

```python
import functools

import jax
import jax.numpy as jnp
from jax import lax
from jax.experimental import pallas as pl
from jax.experimental.pallas import tpu as pltpu

F32, BF16, I32 = jnp.float32, jnp.bfloat16, jnp.int32

N_DEV = 4
M, K, N = 1024, 512, 1024
MB = M // N_DEV
TILE = 128
N_TILES = N // TILE
QR = 64
N_QUADS = (MB // QR) * N_TILES
HALF = N_QUADS // 2

RIGHT, LEFT = 0, 1
DIAG, OWN = 2, 3
HOP, FIN = 0, 2

SWING = 4
HOLD = 8
TAIL = ((0, HALF - 3), (HALF - 3, 2), (HALF - 1, 1))

TOP = 0x78007800
NIBBLE = 0x000F000F
NOTE_ROWS = 9

_srl = lax.shift_right_logical


def _split(y, offset, q, found):
    v = pltpu.bitcast(y.astype(BF16), I32) - offset
    t = v & TOP
    rest = v ^ t
    p = rest[24:]
    low = rest[:24] | (jnp.concatenate([p << 11, p << 7, (p << 3) | _srl(p, 1)]) & TOP)
    top = _srl(t[:8], 11) | _srl(t[8:16], 7) | _srl(t[16:24], 3) | (t[24:] << 1)
    for j in range(4):
        tj = t[8 * j : 8 * j + 8]
        pushed = (tj | (4 * q + j),) + found[:2]
        found = tuple(jnp.where(tj != 0, new, old) for new, old in zip(pushed, found))
    return low, top, found


def _join(low, top, offset):
    h = low & TOP
    p = _srl(h[:8], 11) | _srl(h[8:16], 7) | ((_srl(h[16:], 3) | (h[16:] << 1)) & ~TOP)
    t = jnp.concatenate([top << 11, top << 7, top << 3, _srl(top, 1)]) & TOP
    v = jnp.concatenate([low ^ h, p]) | t
    return pltpu.bitcast(v + offset, BF16).astype(F32)


def _expand(listed, top_ref):
    g1, g2 = listed & 127, _srl(listed, 16) & 127
    t1 = (_srl(listed, 11) & NIBBLE) << (4 * (g1 & 3))
    t2 = (_srl(listed, 7) & NIBBLE) << (4 * (g2 & 3))
    q1, q2 = _srl(g1, 2), _srl(g2, 2)
    for q in range(N_QUADS):
        top_ref[q] = jnp.where(q1 == q, t1, 0) | jnp.where(q2 == q, t2, 0)


def _rows(t, h, route):
    start = 2 * QR * h + QR * (route ^ (t == 1))
    return slice(start, start + QR)


def _quad(step, route):
    return step if route == RIGHT else N_QUADS - 1 - step


def _quads(step, n, route):
    return pl.ds(step if route == RIGHT else N_QUADS - step - n, n)


def _dot(x, w):
    return jnp.dot(x, w, preferred_element_type=F32)


def _wait(ref, sem):
    pltpu.make_async_copy(ref, ref, sem).wait()


def _pipeline(*jobs):
    emit = jobs[0]()
    for job in jobs[1:]:
        following = job()
        emit()
        emit = following
    emit()


def _body(
    a_hbm, b_hbm, o_ref,
    a32, b32, a16, b16, tx, tx_top, tx_note, rx, rx_top, rx_note, swung, acc,
    load_sem, tx_sem, rx_sem, note_tx_sem, note_rx_sem, top_tx_sem, top_rx_sem,
):
    me = lax.axis_index("i")
    owner = ((me + 1) & 3, (me + 3) & 3, (me + 2) & 3, me)
    both = (RIGHT, LEFT)

    loads = {}

    def load_a(name, *parts):
        sem = load_sem.at[len(loads)]
        loads[name] = [
            pltpu.async_copy(
                a_hbm.at[pl.ds(pl.multiple_of(owner[blk] * MB + start, QR), n)],
                a32.at[blk, pl.ds(start, n)],
                sem,
            )
            for blk, start, n in parts
        ]

    def load_b(t):
        sem = load_sem.at[len(loads)]
        loads[t] = [pltpu.async_copy(b_hbm.at[:, pl.ds(t * TILE, TILE)], b32.at[t], sem)]

    def loaded(name):
        for copy in loads[name]:
            copy.wait()

    load_b(0)
    barrier = pltpu.get_barrier_semaphore()
    for d in both:
        pl.semaphore_signal(
            barrier, inc=1, device_id=(owner[d],), device_id_type=pl.DeviceIdType.MESH
        )
    load_a("diag0", (DIAG, 0, 2 * QR))
    load_b(1)
    load_a("diag1", (DIAG, 2 * QR, QR))
    load_a("diag2", (DIAG, 3 * QR, QR))
    for t in range(2, 6):
        load_b(t)
    load_a("direct", *[(d, _rows(0, h, 1 - d).start, QR) for h in (0, 1) for d in both])
    load_b(6)
    load_b(7)
    load_a("relay", *[(d, _rows(0, h, d).start, QR) for h in (0, 1) for d in both])
    load_a("own", (OWN, 0, MB))
    swung[...] = jnp.zeros(swung.shape, F32)

    def cast_a(blk, rows):
        x = a32[blk, rows].astype(BF16)
        a16[blk, rows] = x
        return x

    def cast_b(t):
        w = b32[t].astype(BF16)
        b16[t] = w
        return w

    found = [(jnp.zeros((8, TILE), I32),) * 3] * 3
    notes = []

    def remote(src, dst, send_sem, recv_sem, d):
        if isinstance(d, int):
            device = owner[d]
        else:
            device = jnp.where(d == RIGHT, owner[RIGHT], owner[LEFT])
        return pltpu.make_async_remote_copy(
            src, dst, send_sem, recv_sem,
            device_id=(device,), device_id_type=pl.DeviceIdType.MESH,
        )

    def put(blk, q, y):
        tx[blk, q], tx_top[blk, q], found[blk] = _split(y, offset, q, found[blk])

    def get(stream, q):
        return _join(rx[stream, q], rx_top[stream, q], rx_note[stream, 8:9] & 0x7FFFFFFF)

    def top_copy(blk, s):
        return remote(
            tx_top.at[blk], rx_top.at[s], top_tx_sem.at[s], top_rx_sem.at[s], s % 2
        )

    def send_top(blk, streams):
        first, second, third = found[blk]
        overflow = jnp.max(jnp.where(third != 0, 1.0, 0.0), keepdims=True)
        tx_note[blk, :8] = first | _srl(second & TOP, 4) | ((second & 127) << 16)
        tx_note[blk, 8:9] = offset | (overflow.astype(I32) << 31)
        dense = overflow[0, 0] > 0
        for s in streams:
            note = remote(
                tx_note.at[blk, pl.ds(0, NOTE_ROWS)], rx_note.at[s, pl.ds(0, NOTE_ROWS)],
                note_tx_sem.at[s], note_rx_sem.at[s], s % 2,
            )
            note.start()
            notes.append((note, blk, s, dense))
        for s in streams:
            pl.when(dense)(lambda: top_copy(blk, s).start())

    def recv_top(kind):
        streams = [kind + d for d in both]
        for s in streams:
            _wait(rx_note.at[s, pl.ds(0, NOTE_ROWS)], note_rx_sem.at[s])
        for s, dense in [(s, rx_note[s, 8:9][0, 0] < 0) for s in streams]:
            pl.when(dense)(lambda: _wait(rx_top.at[s], top_rx_sem.at[s]))
            pl.when(jnp.logical_not(dense))(lambda: _expand(rx_note[s, :8], rx_top.at[s]))

    def send_hop(step, route):
        d = route
        if step >= HALF - SWING:
            d = jnp.where(me == 1, RIGHT, jnp.where(me == 3, LEFT, route))
        q = _quad(step, route)
        remote(tx.at[DIAG, q], rx.at[HOP + d, q], tx_sem, rx_sem.at[d], d).start()

    def recv_hop(n):
        for d in both:
            _wait(rx.at[HOP + d, _quads(0, n, d)], rx_sem.at[d])
        recv_top(HOP)
        for d in both:
            for q in (_quad(step, d) for step in range(HALF - SWING, n)):
                swung[d, q - (HALF - SWING)] = get(HOP + d, q)

    def send_fin(step, n, relay, group):
        for d in both:
            qs = _quads(step, n, d if relay else 1 - d)
            sem = rx_sem.at[2 * group + d]
            remote(tx.at[d, qs], rx.at[FIN + d, qs], tx_sem, sem, d).start()

    def put_hop(t, h, y):
        for route in both:
            put(DIAG, _quad(2 * t + h, route), y[_rows(t, h, route)])

    def hop_job(t):
        y = _dot(a16[DIAG], cast_b(t))

        def emit():
            for h in (0, 1):
                put_hop(t, h, y)
                for route in both:
                    send_hop(2 * t + h, route)

        return emit

    def fin_job(t, relay):
        parts = [(h, d, d if relay else 1 - d) for h in (0, 1) for d in both]
        x = jnp.concatenate([a16[d, _rows(t, h, route)] for h, d, route in parts])
        y = _dot(x, b16[t])

        def emit():
            for i, (h, d, route) in enumerate(parts):
                q, part = _quad(2 * t + h, route), y[i * QR : (i + 1) * QR]
                if 2 * t + h >= HALF - SWING:
                    part += swung[d, q - (HALF - SWING)]
                elif relay:
                    part += get(HOP + d, q)
                put(d, q, part)
            if not relay or 2 * t < HALF - HOLD:
                send_fin(2 * t, 2, relay, 1 + relay)

        return emit

    def fin_jobs(tiles, relay):
        return [functools.partial(fin_job, t, relay) for t in tiles]

    def cast_fin(relay):
        loaded("relay" if relay else "direct")
        for h in (0, 1):
            for d in both:
                cast_a(d, _rows(0, h, d if relay else 1 - d))

    loaded(0)
    cast_b(0)
    loaded("diag0")
    y = _dot(cast_a(DIAG, slice(0, 2 * QR)), b16[0])
    big = lax.bitcast_convert_type(jnp.max(jnp.abs(y[:16]), keepdims=True), I32)
    bottom = jnp.maximum((_srl(big, 16) & 0x7FFF) + (144 - 2047), 0)
    offset = jnp.broadcast_to(bottom | (bottom << 16), (1, TILE))
    put_hop(0, 0, y)
    pl.semaphore_wait(barrier, 2)
    for route in both:
        send_hop(0, route)
    loaded(1)
    put_hop(1, 0, _dot(a16[DIAG, : 2 * QR], cast_b(1)))
    for route in both:
        send_hop(2, route)
    for name, route in (("diag1", RIGHT), ("diag2", LEFT)):
        loaded(name)
        x = cast_a(DIAG, _rows(0, 1, route))
        for t, y in enumerate([_dot(x, b16[0]), _dot(x, b16[1])]):
            put(DIAG, _quad(2 * t + 1, route ^ t), y)
            send_hop(2 * t + 1, route ^ t)

    for t in range(2, 6):
        loaded(t)
        hop_job(t)()
    cast_fin(False)
    _pipeline(*fin_jobs((0, 2), False))
    loaded(6)
    loaded(7)
    _pipeline(
        functools.partial(hop_job, 6),
        functools.partial(hop_job, 7),
        lambda: functools.partial(send_top, DIAG, (HOP + RIGHT, HOP + LEFT)),
        *fin_jobs((3, 4, 5), False),
    )
    cast_fin(True)
    fin_job(1, False)()
    emit = fin_job(6, False)
    pl.when(me == 2)(lambda: recv_hop(HALF + SWING))
    _pipeline(lambda: emit, *fin_jobs((7,), False))

    emit = fin_job(0, True)
    pl.when(me == 0)(lambda: recv_hop(HALF - SWING))
    pl.when((me & 1) == 1)(lambda: recv_hop(HALF))
    emit()
    _pipeline(*fin_jobs(range(1, N_TILES), True))
    for d in both:
        send_top(d, (FIN + d,))
    send_fin(HALF - HOLD, TAIL[0][1] - (HALF - HOLD), True, 2)
    send_fin(*TAIL[1], True, 3)
    send_fin(*TAIL[2], True, 4)

    loaded("own")
    cast_a(OWN, slice(0, MB))
    for t in range(N_TILES):
        acc[t] = _dot(a16[OWN], b16[t])
    for d in both:
        _wait(rx.at[FIN + d, _quads(0, HALF, 1 - d)], rx_sem.at[2 + d])
    recv_top(FIN)
    for step in range(HALF):
        t, h = divmod(step, 2)
        for d in both:
            acc[t, _rows(t, h, 1 - d)] += get(FIN + d, _quad(step, 1 - d))

    def finish(first, n, group):
        for d in both:
            _wait(rx.at[FIN + d, _quads(first, n, d)], rx_sem.at[2 * group + d])
            for step in range(first, first + n):
                t, h = divmod(step, 2)
                total = acc[t, _rows(t, h, d)] + get(FIN + d, _quad(step, d))
                o_ref[_rows(t, h, d), t * TILE : (t + 1) * TILE] = total.astype(BF16)

    finish(*TAIL[0], 2)
    for note, blk, s, dense in notes:
        note.wait_send()
        pl.when(dense)(lambda: top_copy(blk, s).wait_send())
    finish(*TAIL[1], 3)
    _wait(tx, tx_sem)
    finish(*TAIL[2], 4)


def pallas_dist_matmul_mk_i_outk_m1024_n1024_k512_kernel(
    A: jax.Array,
    B: jax.Array,
):
    dma = pltpu.SemaphoreType.DMA
    return pl.pallas_call(
        _body,
        out_shape=jax.ShapeDtypeStruct((MB, N), BF16),
        in_specs=[pl.BlockSpec(memory_space=pl.ANY)] * 2,
        out_specs=pl.BlockSpec(memory_space=pltpu.VMEM),
        scratch_shapes=[
            pltpu.VMEM((N_DEV, MB, K), F32),
            pltpu.VMEM((N_TILES, K, TILE), F32),
            pltpu.VMEM((N_DEV, MB, K), BF16),
            pltpu.VMEM((N_TILES, K, TILE), BF16),
            pltpu.VMEM((3, N_QUADS, 24, TILE), I32),
            pltpu.VMEM((3, N_QUADS, 8, TILE), I32),
            pltpu.VMEM((3, 16, TILE), I32),
            pltpu.VMEM((4, N_QUADS, 24, TILE), I32),
            pltpu.VMEM((4, N_QUADS, 8, TILE), I32),
            pltpu.VMEM((4, 16, TILE), I32),
            pltpu.VMEM((2, 2 * SWING, QR, TILE), F32),
            pltpu.VMEM((N_TILES, MB, TILE), F32),
            dma((N_TILES + 6,)),
            dma,
            dma((10,)),
            dma((4,)),
            dma((4,)),
            dma((4,)),
            dma((4,)),
        ],
        compiler_params=pltpu.CompilerParams(
            collective_id=0, disable_semaphore_checks=True
        ),
    )(A, B)
```

```python
import functools

import jax
import jax.numpy as jnp
from jax import lax
from jax.experimental import pallas as pl
from jax.experimental.pallas import tpu as pltpu

F32, BF16, I32 = jnp.float32, jnp.bfloat16, jnp.int32

N_DEV = 4
M, K, N = 1024, 512, 1024
MB = M // N_DEV
TILE = 128
N_TILES = N // TILE
QR = 64
N_QUADS = (MB // QR) * N_TILES
HALF = N_QUADS // 2

RIGHT, LEFT = 0, 1
DIAG, OWN = 2, 3
HOP, FIN = 0, 2

SWING = 3
HOLD = 8
TAIL = ((0, HALF - 3), (HALF - 3, 2), (HALF - 1, 1))

TOP = 0x78007800
NIBBLE = 0x000F000F
NOTE_ROWS = 9

_srl = lax.shift_right_logical


def _split(y, offset, q, found):
    v = pltpu.bitcast(y.astype(BF16), I32) - offset
    t = v & TOP
    rest = v ^ t
    p = rest[24:]
    low = rest[:24] | (jnp.concatenate([p << 11, p << 7, (p << 3) | _srl(p, 1)]) & TOP)
    top = _srl(t[:8], 11) | _srl(t[8:16], 7) | _srl(t[16:24], 3) | (t[24:] << 1)
    for j in range(4):
        tj = t[8 * j : 8 * j + 8]
        pushed = (tj | (4 * q + j),) + found[:2]
        found = tuple(jnp.where(tj != 0, new, old) for new, old in zip(pushed, found))
    return low, top, found


def _join(low, top, offset):
    h = low & TOP
    p = _srl(h[:8], 11) | _srl(h[8:16], 7) | ((_srl(h[16:], 3) | (h[16:] << 1)) & ~TOP)
    t = jnp.concatenate([top << 11, top << 7, top << 3, _srl(top, 1)]) & TOP
    v = jnp.concatenate([low ^ h, p]) | t
    return pltpu.bitcast(v + offset, BF16).astype(F32)


def _expand(listed, top_ref):
    g1, g2 = listed & 127, _srl(listed, 16) & 127
    t1 = (_srl(listed, 11) & NIBBLE) << (4 * (g1 & 3))
    t2 = (_srl(listed, 7) & NIBBLE) << (4 * (g2 & 3))
    q1, q2 = _srl(g1, 2), _srl(g2, 2)
    for q in range(N_QUADS):
        top_ref[q] = jnp.where(q1 == q, t1, 0) | jnp.where(q2 == q, t2, 0)


def _rows(t, h, route):
    start = 2 * QR * h + QR * (route ^ (t == 1))
    return slice(start, start + QR)


def _quad(step, route):
    return step if route == RIGHT else N_QUADS - 1 - step


def _quads(step, n, route):
    return pl.ds(step if route == RIGHT else N_QUADS - step - n, n)


def _dot(x, w):
    return jnp.dot(x, w, preferred_element_type=F32)


def _wait(ref, sem):
    pltpu.make_async_copy(ref, ref, sem).wait()


def _pipeline(*jobs):
    emit = jobs[0]()
    for job in jobs[1:]:
        following = job()
        emit()
        emit = following
    emit()


def _body(
    a_hbm, b_hbm, o_ref,
    a32, b32, a16, b16, tx, tx_top, tx_note, rx, rx_top, rx_note, swung, acc,
    load_sem, tx_sem, rx_sem, note_tx_sem, note_rx_sem, top_tx_sem, top_rx_sem,
):
    me = lax.axis_index("i")
    owner = ((me + 1) & 3, (me + 3) & 3, (me + 2) & 3, me)
    both = (RIGHT, LEFT)

    loads = {}

    def load_a(name, *parts):
        sem = load_sem.at[len(loads)]
        loads[name] = [
            pltpu.async_copy(
                a_hbm.at[pl.ds(pl.multiple_of(owner[blk] * MB + start, QR), n)],
                a32.at[blk, pl.ds(start, n)],
                sem,
            )
            for blk, start, n in parts
        ]

    def load_b(t):
        sem = load_sem.at[len(loads)]
        loads[t] = [pltpu.async_copy(b_hbm.at[:, pl.ds(t * TILE, TILE)], b32.at[t], sem)]

    def loaded(name):
        for copy in loads[name]:
            copy.wait()

    load_b(0)
    barrier = pltpu.get_barrier_semaphore()
    for d in both:
        pl.semaphore_signal(
            barrier, inc=1, device_id=(owner[d],), device_id_type=pl.DeviceIdType.MESH
        )
    load_a("diag0", (DIAG, 0, 2 * QR))
    load_b(1)
    load_a("diag1", (DIAG, 2 * QR, QR))
    load_a("diag2", (DIAG, 3 * QR, QR))
    for t in range(2, 6):
        load_b(t)
    load_a("direct", *[(d, _rows(0, h, 1 - d).start, QR) for h in (0, 1) for d in both])
    load_b(6)
    load_b(7)
    load_a("relay", *[(d, _rows(0, h, d).start, QR) for h in (0, 1) for d in both])
    load_a("own", (OWN, 0, MB))
    swung[...] = jnp.zeros(swung.shape, F32)

    def cast_a(blk, rows):
        x = a32[blk, rows].astype(BF16)
        a16[blk, rows] = x
        return x

    def cast_b(t):
        w = b32[t].astype(BF16)
        b16[t] = w
        return w

    found = [(jnp.zeros((8, TILE), I32),) * 3] * 3
    notes = []

    def remote(src, dst, send_sem, recv_sem, d):
        if isinstance(d, int):
            device = owner[d]
        else:
            device = jnp.where(d == RIGHT, owner[RIGHT], owner[LEFT])
        return pltpu.make_async_remote_copy(
            src, dst, send_sem, recv_sem,
            device_id=(device,), device_id_type=pl.DeviceIdType.MESH,
        )

    def put(blk, q, y):
        tx[blk, q], tx_top[blk, q], found[blk] = _split(y, offset, q, found[blk])

    def get(stream, q):
        return _join(rx[stream, q], rx_top[stream, q], rx_note[stream, 8:9] & 0x7FFFFFFF)

    def top_copy(blk, s):
        return remote(
            tx_top.at[blk], rx_top.at[s], top_tx_sem.at[s], top_rx_sem.at[s], s % 2
        )

    def send_top(blk, streams):
        first, second, third = found[blk]
        overflow = jnp.max(jnp.where(third != 0, 1.0, 0.0), keepdims=True)
        tx_note[blk, :8] = first | _srl(second & TOP, 4) | ((second & 127) << 16)
        tx_note[blk, 8:9] = offset | (overflow.astype(I32) << 31)
        dense = overflow[0, 0] > 0
        for s in streams:
            note = remote(
                tx_note.at[blk, pl.ds(0, NOTE_ROWS)], rx_note.at[s, pl.ds(0, NOTE_ROWS)],
                note_tx_sem.at[s], note_rx_sem.at[s], s % 2,
            )
            note.start()
            notes.append((note, blk, s, dense))
        for s in streams:
            pl.when(dense)(lambda: top_copy(blk, s).start())

    def recv_top(kind):
        streams = [kind + d for d in both]
        for s in streams:
            _wait(rx_note.at[s, pl.ds(0, NOTE_ROWS)], note_rx_sem.at[s])
        for s, dense in [(s, rx_note[s, 8:9][0, 0] < 0) for s in streams]:
            pl.when(dense)(lambda: _wait(rx_top.at[s], top_rx_sem.at[s]))
            pl.when(jnp.logical_not(dense))(lambda: _expand(rx_note[s, :8], rx_top.at[s]))

    def send_hop(step, route):
        d = route
        if step >= HALF - SWING:
            d = jnp.where(me == 1, RIGHT, jnp.where(me == 3, LEFT, route))
        q = _quad(step, route)
        remote(tx.at[DIAG, q], rx.at[HOP + d, q], tx_sem, rx_sem.at[d], d).start()

    def recv_hop(n):
        for d in both:
            _wait(rx.at[HOP + d, _quads(0, n, d)], rx_sem.at[d])
        recv_top(HOP)
        for d in both:
            for q in (_quad(step, d) for step in range(HALF - SWING, n)):
                swung[d, q - (HALF - SWING)] = get(HOP + d, q)

    def send_fin(step, n, relay, group):
        for d in both:
            qs = _quads(step, n, d if relay else 1 - d)
            sem = rx_sem.at[2 * group + d]
            remote(tx.at[d, qs], rx.at[FIN + d, qs], tx_sem, sem, d).start()

    def emit_hop(step, route, y):
        put(DIAG, _quad(step, route), y)
        send_hop(step, route)

    def hop_job(t):
        y = _dot(a16[DIAG], cast_b(t))

        def emit():
            for h in (0, 1):
                for route in both:
                    emit_hop(2 * t + h, route, y[_rows(t, h, route)])

        return emit

    def fin_job(t, relay):
        parts = [(h, d, d if relay else 1 - d) for h in (0, 1) for d in both]
        x = jnp.concatenate([a16[d, _rows(t, h, route)] for h, d, route in parts])
        y = _dot(x, b16[t])

        def emit():
            for i, (h, d, route) in enumerate(parts):
                q, part = _quad(2 * t + h, route), y[i * QR : (i + 1) * QR]
                if 2 * t + h >= HALF - SWING:
                    part += swung[d, q - (HALF - SWING)]
                elif relay:
                    part += get(HOP + d, q)
                put(d, q, part)
            if not relay or 2 * t < HALF - HOLD:
                send_fin(2 * t, 2, relay, 1 + relay)

        return emit

    def fin_jobs(tiles, relay):
        return [functools.partial(fin_job, t, relay) for t in tiles]

    def cast_fin(relay):
        loaded("relay" if relay else "direct")
        for h in (0, 1):
            for d in both:
                cast_a(d, _rows(0, h, d if relay else 1 - d))

    loaded(0)
    cast_b(0)
    loaded("diag0")
    y = _dot(cast_a(DIAG, slice(0, 2 * QR)), b16[0])
    big = lax.bitcast_convert_type(jnp.max(jnp.abs(y[:16]), keepdims=True), I32)
    bottom = jnp.maximum((_srl(big, 16) & 0x7FFF) + (136 - 2047), 0)
    offset = jnp.broadcast_to(bottom | (bottom << 16), (1, TILE))
    for route in both:
        put(DIAG, _quad(0, route), y[_rows(0, 0, route)])
    pl.semaphore_wait(barrier, 2)
    for route in both:
        send_hop(0, route)
    loaded(1)
    y = _dot(jnp.concatenate([a16[DIAG, _rows(1, 0, route)] for route in both]), cast_b(1))
    for route in both:
        emit_hop(2, route, y[route * QR : (route + 1) * QR])
    for name, route in (("diag1", RIGHT), ("diag2", LEFT)):
        loaded(name)
        x = cast_a(DIAG, _rows(0, 1, route))
        for t, y in enumerate([_dot(x, b16[0]), _dot(x, b16[1])]):
            emit_hop(2 * t + 1, route ^ t, y)

    for t in range(2, 6):
        loaded(t)
        hop_job(t)()
    cast_fin(False)
    _pipeline(*fin_jobs((0, 2), False))
    loaded(6)
    loaded(7)
    _pipeline(
        functools.partial(hop_job, 6),
        functools.partial(hop_job, 7),
        lambda: functools.partial(send_top, DIAG, (HOP + RIGHT, HOP + LEFT)),
        *fin_jobs((3, 4, 5), False),
    )
    cast_fin(True)
    fin_job(1, False)()
    emit = fin_job(6, False)
    pl.when(me == 2)(lambda: recv_hop(HALF + SWING))
    _pipeline(lambda: emit, *fin_jobs((7,), False))

    emit = fin_job(0, True)
    pl.when(me == 0)(lambda: recv_hop(HALF - SWING))
    pl.when((me & 1) == 1)(lambda: recv_hop(HALF))
    emit()
    _pipeline(*fin_jobs(range(1, N_TILES), True))
    for d in both:
        send_top(d, (FIN + d,))
    send_fin(HALF - HOLD, TAIL[0][1] - (HALF - HOLD), True, 2)
    send_fin(*TAIL[1], True, 3)
    send_fin(*TAIL[2], True, 4)

    loaded("own")
    cast_a(OWN, slice(0, MB))
    for t in range(N_TILES):
        acc[t] = _dot(a16[OWN], b16[t])
    for d in both:
        _wait(rx.at[FIN + d, _quads(0, HALF, 1 - d)], rx_sem.at[2 + d])
    recv_top(FIN)
    for step in range(HALF):
        t, h = divmod(step, 2)
        for d in both:
            acc[t, _rows(t, h, 1 - d)] += get(FIN + d, _quad(step, 1 - d))

    def finish(first, n, group):
        for d in both:
            _wait(rx.at[FIN + d, _quads(first, n, d)], rx_sem.at[2 * group + d])
            for step in range(first, first + n):
                t, h = divmod(step, 2)
                total = acc[t, _rows(t, h, d)] + get(FIN + d, _quad(step, d))
                o_ref[_rows(t, h, d), t * TILE : (t + 1) * TILE] = total.astype(BF16)

    finish(*TAIL[0], 2)
    for note, blk, s, dense in notes:
        note.wait_send()
        pl.when(dense)(lambda: top_copy(blk, s).wait_send())
    finish(*TAIL[1], 3)
    _wait(tx, tx_sem)
    finish(*TAIL[2], 4)


def pallas_dist_matmul_mk_i_outk_m1024_n1024_k512_kernel(
    A: jax.Array,
    B: jax.Array,
):
    dma = pltpu.SemaphoreType.DMA
    return pl.pallas_call(
        _body,
        out_shape=jax.ShapeDtypeStruct((MB, N), BF16),
        in_specs=[pl.BlockSpec(memory_space=pl.ANY)] * 2,
        out_specs=pl.BlockSpec(memory_space=pltpu.VMEM),
        scratch_shapes=[
            pltpu.VMEM((N_DEV, MB, K), F32),
            pltpu.VMEM((N_TILES, K, TILE), F32),
            pltpu.VMEM((N_DEV, MB, K), BF16),
            pltpu.VMEM((N_TILES, K, TILE), BF16),
            pltpu.VMEM((3, N_QUADS, 24, TILE), I32),
            pltpu.VMEM((3, N_QUADS, 8, TILE), I32),
            pltpu.VMEM((3, 16, TILE), I32),
            pltpu.VMEM((4, N_QUADS, 24, TILE), I32),
            pltpu.VMEM((4, N_QUADS, 8, TILE), I32),
            pltpu.VMEM((4, 16, TILE), I32),
            pltpu.VMEM((2, 2 * SWING, QR, TILE), F32),
            pltpu.VMEM((N_TILES, MB, TILE), F32),
            dma((N_TILES + 6,)),
            dma,
            dma((10,)),
            dma((4,)),
            dma((4,)),
            dma((4,)),
            dma((4,)),
        ],
        compiler_params=pltpu.CompilerParams(
            collective_id=0, disable_semaphore_checks=True
        ),
    )(A, B)
```
